```python
import numpy as np

kernel_name = "dist_mean_ax0_shard0_i_m1024_n512"

def setup_inputs():
    return {"x": np.random.randn(4096, 512).astype(np.float32)}

def reference(x: np.ndarray) -> np.ndarray:
    return np.mean(x, axis=0, keepdims=True)
```

```python
import jax
import jax.numpy as jnp
from jax import lax
from jax.experimental import pallas as pl
from jax.experimental.pallas import tpu as pltpu

N_DEV = 4
N_CHUNK = 8


def pallas_dist_mean_ax0_shard0_i_m1024_n512_kernel(
    x: jax.Array,
):
    m, n = x.shape
    rows = m // N_CHUNK
    inv_total = 1.0 / float(m * N_DEV)

    def kernel_body(x_hbm, out_ref, xbuf, comm, load_sems, send_sems, recv_sems):
        my = lax.axis_index("i")

        loads = [
            pltpu.make_async_copy(
                x_hbm.at[pl.ds(c * rows, rows), :],
                xbuf.at[pl.ds(c * rows, rows), :],
                load_sems.at[c],
            )
            for c in range(N_CHUNK)
        ]
        for cp in loads:
            cp.start()

        barrier = pltpu.get_barrier_semaphore()
        for d in range(1, N_DEV):
            pl.semaphore_signal(
                barrier,
                inc=1,
                device_id=((my + d) % N_DEV,),
                device_id_type=pl.DeviceIdType.MESH,
            )

        acc = jnp.zeros((8, n), jnp.float32)
        for c in range(N_CHUNK):
            loads[c].wait()
            blk = xbuf[pl.ds(c * rows, rows), :]
            acc = acc + jnp.sum(blk.reshape(rows // 8, 8, n), axis=0)
        part = jnp.sum(acc, axis=0, keepdims=True)
        comm[0] = part

        pl.semaphore_wait(barrier, N_DEV - 1)

        rdmas = []
        for d in range(1, N_DEV):
            r = pltpu.make_async_remote_copy(
                src_ref=comm.at[0],
                dst_ref=comm.at[d],
                send_sem=send_sems.at[d - 1],
                recv_sem=recv_sems.at[d - 1],
                device_id=((my + d) % N_DEV,),
                device_id_type=pl.DeviceIdType.MESH,
            )
            r.start()
            rdmas.append(r)

        tot = part
        for d in range(1, N_DEV):
            rdmas[d - 1].wait_recv()
            tot = tot + comm[d]
        out_ref[...] = tot * inv_total
        for r in rdmas:
            r.wait_send()

    return pl.pallas_call(
        kernel_body,
        out_shape=jax.ShapeDtypeStruct((1, n), jnp.float32),
        in_specs=[pl.BlockSpec(memory_space=pl.ANY)],
        out_specs=pl.BlockSpec(memory_space=pltpu.VMEM),
        scratch_shapes=[
            pltpu.VMEM((m, n), jnp.float32),
            pltpu.VMEM((N_DEV, 1, n), jnp.float32),
            pltpu.SemaphoreType.DMA((N_CHUNK,)),
            pltpu.SemaphoreType.DMA((N_DEV - 1,)),
            pltpu.SemaphoreType.DMA((N_DEV - 1,)),
        ],
        compiler_params=pltpu.CompilerParams(collective_id=0),
    )(x)
```

```python
import jax
import jax.numpy as jnp
from jax import lax
from jax.experimental import pallas as pl
from jax.experimental.pallas import tpu as pltpu

N_DEV = 4
LANES = 128
SUB = 8
MESH = pl.DeviceIdType.MESH

MAIN_CHUNKS = (256, 256, 256, 128, 64)


def _tree_sum(vs):
    vs = list(vs)
    while len(vs) > 1:
        nxt = [vs[i] + vs[i + 1] for i in range(0, len(vs) - 1, 2)]
        if len(vs) % 2:
            nxt.append(vs[-1])
        vs = nxt
    return vs[0]


def _compiler_params():
    try:
        return pltpu.CompilerParams(collective_id=0, disable_semaphore_checks=True)
    except TypeError:
        return pltpu.CompilerParams(collective_id=0)


def pallas_dist_mean_ax0_shard0_i_m1024_n512_kernel(
    x: jax.Array,
):
    m, n = x.shape
    ncb = n // LANES
    assert ncb == 4 and n == ncb * LANES
    main = MAIN_CHUNKS
    r1 = sum(main)
    nt = (m - r1) // SUB
    assert r1 + nt * SUB == m and nt >= 2
    offs = [sum(main[:i]) for i in range(len(main))]
    inv_total = 1.0 / float(m * N_DEV)
    n_load = len(main) + 3

    def body(x_hbm, out_ref, xbuf, full, bulk, outer, mid,
             recv_sems, load_sems, send_sems):
        def load(r, nr, cb, ncols, sem):
            sl = (pl.ds(r, nr), pl.ds(cb * LANES, ncols * LANES))
            return pltpu.make_async_copy(x_hbm.at[sl], xbuf.at[sl], load_sems.at[sem])

        g_main = [load(o, r, 0, ncb, c) for c, (o, r) in enumerate(zip(offs, main))]
        g_outer = []
        for t in range(nt):
            g_outer += [
                load(r1 + SUB * t, SUB, 0, 1, len(main)),
                load(r1 + SUB * t, SUB, 3, 1, len(main)),
            ]
        g_mid0 = load(r1, (nt - 1) * SUB, 1, 2, len(main) + 1)
        g_mid1 = load(m - SUB, SUB, 1, 2, len(main) + 2)
        for cp in g_main + g_outer + [g_mid0, g_mid1]:
            cp.start()

        my = lax.axis_index("i")
        right = lax.rem(my + 1, N_DEV)
        diag = lax.rem(my + 2, N_DEV)
        left = lax.rem(my + 3, N_DEV)

        barrier = pltpu.get_barrier_semaphore()
        for peer in (diag, right, left):
            pl.semaphore_signal(barrier, inc=1, device_id=(peer,), device_id_type=MESH)

        def remote(k, src, dst, peer):
            return pltpu.make_async_remote_copy(
                src_ref=src, dst_ref=dst,
                send_sem=send_sems.at[k], recv_sem=recv_sems.at[k],
                device_id=(peer,), device_id_type=MESH)

        cps = [
            remote(0, bulk.at[0], bulk.at[1], diag),
            remote(1, outer.at[0], outer.at[1], diag),
            remote(2, mid.at[0], mid.at[1], diag),
            remote(3, full.at[0], full.at[1], right),
            remote(4, full.at[0], full.at[2], left),
        ]

        def tile(t, cb):
            return xbuf[pl.ds(r1 + SUB * t, SUB), pl.ds(cb * LANES, LANES)]

        def fold(v):
            return jnp.sum(v, axis=0, keepdims=True) * inv_total

        acc = None
        for c, (o, r) in enumerate(zip(offs, main)):
            if c == len(main) - 1:
                pl.semaphore_wait(barrier, N_DEV - 1)
            g_main[c].wait()
            s = jnp.sum(xbuf[pl.ds(o, r), :].reshape(r // SUB, SUB, n), axis=0)
            acc = s if acc is None else acc + s
        b = [fold(acc[:, cb * LANES:(cb + 1) * LANES]) for cb in range(ncb)]
        bulk[0] = jnp.concatenate(b, axis=0)
        cps[0].start()

        for cp in g_outer:
            cp.wait()
        t0 = fold(_tree_sum([tile(t, 0) for t in range(nt)]))
        t3 = fold(_tree_sum([tile(t, 3) for t in range(nt)]))
        outer[0] = jnp.concatenate([t0, t3], axis=0).astype(outer.dtype)
        cps[1].start()

        g_mid0.wait()
        a1 = _tree_sum([tile(t, 1) for t in range(nt - 1)])
        a2 = _tree_sum([tile(t, 2) for t in range(nt - 1)])
        g_mid1.wait()
        t1 = fold(a1 + tile(nt - 1, 1))
        t2 = fold(a2 + tile(nt - 1, 2))
        mid[0] = jnp.concatenate([t1, t2], axis=0).astype(mid.dtype)
        cps[2].start()

        full[0] = jnp.concatenate(
            [b[0] + t0, b[1] + t1, b[2] + t2, b[3] + t3], axis=0)
        cps[3].start()
        cps[4].start()
        for cp in cps:
            cp.wait_send()

        cps[3].wait_recv()
        cps[4].wait_recv()
        cps[0].wait_recv()
        out_ref[...] = (full[0] + full[1]) + (full[2] + bulk[1])
        p0 = out_ref[pl.ds(0, 1), :]
        p3 = out_ref[pl.ds(3, 1), :]
        pm = out_ref[pl.ds(1, 2), :]
        cps[1].wait_recv()
        v = outer[1].astype(jnp.float32)
        out_ref[pl.ds(0, 1), :] = p0 + v[0:1, :]
        out_ref[pl.ds(3, 1), :] = p3 + v[1:2, :]
        cps[2].wait_recv()
        out_ref[pl.ds(1, 2), :] = pm + mid[1].astype(jnp.float32)

    out = pl.pallas_call(
        body,
        out_shape=jax.ShapeDtypeStruct((ncb, LANES), jnp.float32),
        in_specs=[pl.BlockSpec(memory_space=pl.ANY)],
        out_specs=pl.BlockSpec(memory_space=pltpu.VMEM),
        scratch_shapes=[
            pltpu.VMEM((m, n), jnp.float32),
            pltpu.VMEM((3, ncb, LANES), jnp.float32),
            pltpu.VMEM((2, ncb, LANES), jnp.float32),
            pltpu.VMEM((2, 2, LANES), jnp.bfloat16),
            pltpu.VMEM((2, 2, LANES), jnp.bfloat16),
            pltpu.SemaphoreType.DMA((5,)),
            pltpu.SemaphoreType.DMA((n_load,)),
            pltpu.SemaphoreType.DMA((5,)),
        ],
        compiler_params=_compiler_params(),
    )(x)
    return out.reshape(1, n)
```

```python
import jax
import jax.numpy as jnp
from jax import lax
from jax.experimental import pallas as pl
from jax.experimental.pallas import tpu as pltpu

N_DEV = 4
LANES = 128
SUB = 8
MESH = pl.DeviceIdType.MESH

MAIN_CHUNKS = (256, 256, 256, 128, 64)
PAIR_A = (0, 2)
PAIR_B = (1, 3)


def _tree_sum(vs):
    vs = list(vs)
    while len(vs) > 1:
        nxt = [vs[i] + vs[i + 1] for i in range(0, len(vs) - 1, 2)]
        if len(vs) % 2:
            nxt.append(vs[-1])
        vs = nxt
    return vs[0]


def _compiler_params():
    try:
        return pltpu.CompilerParams(collective_id=0, disable_semaphore_checks=True)
    except TypeError:
        return pltpu.CompilerParams(collective_id=0)


def pallas_dist_mean_ax0_shard0_i_m1024_n512_kernel(
    x: jax.Array,
):
    m, n = x.shape
    ncb = n // LANES
    assert ncb == 4 and n == ncb * LANES
    main = MAIN_CHUNKS
    r1 = sum(main)
    nt = (m - r1) // SUB
    assert r1 + nt * SUB == m and nt >= 2
    offs = [sum(main[:i]) for i in range(len(main))]
    inv_total = 1.0 / float(m * N_DEV)
    n_load = len(main) + 3

    def body(x_hbm, out_ref, xbuf, full, bulk, tail_a, tail_b,
             recv_sems, load_sems, send_sems):
        def load(r, nr, cb, ncols, sem):
            sl = (pl.ds(r, nr), pl.ds(cb * LANES, ncols * LANES))
            return pltpu.make_async_copy(x_hbm.at[sl], xbuf.at[sl], load_sems.at[sem])

        def tile_loads(pair, ts, sem):
            return [load(r1 + SUB * t, SUB, cb, 1, sem) for t in ts for cb in pair]

        g_main = [load(o, r, 0, ncb, c) for c, (o, r) in enumerate(zip(offs, main))]
        g_a = tile_loads(PAIR_A, range(nt), len(main))
        g_b0 = tile_loads(PAIR_B, range(nt - 1), len(main) + 1)
        g_b1 = tile_loads(PAIR_B, [nt - 1], len(main) + 2)
        for cp in g_main + g_a + g_b0 + g_b1:
            cp.start()

        my = lax.axis_index("i")
        right = lax.rem(my + 1, N_DEV)
        diag = lax.rem(my + 2, N_DEV)
        left = lax.rem(my + 3, N_DEV)

        barrier = pltpu.get_barrier_semaphore()
        for peer in (diag, right, left):
            pl.semaphore_signal(barrier, inc=1, device_id=(peer,), device_id_type=MESH)

        def remote(k, src, dst, peer):
            return pltpu.make_async_remote_copy(
                src_ref=src, dst_ref=dst,
                send_sem=send_sems.at[k], recv_sem=recv_sems.at[k],
                device_id=(peer,), device_id_type=MESH)

        cps = [
            remote(0, bulk.at[0], bulk.at[1], diag),
            remote(1, tail_a.at[0], tail_a.at[1], diag),
            remote(2, tail_b.at[0], tail_b.at[1], diag),
            remote(3, full.at[0], full.at[1], right),
            remote(4, full.at[0], full.at[2], left),
        ]

        def tile(t, cb):
            return xbuf[pl.ds(r1 + SUB * t, SUB), pl.ds(cb * LANES, LANES)]

        def fold(v):
            return jnp.sum(v, axis=0, keepdims=True) * inv_total

        acc = None
        for c, (o, r) in enumerate(zip(offs, main)):
            if c == len(main) - 1:
                pl.semaphore_wait(barrier, N_DEV - 1)
            g_main[c].wait()
            s = jnp.sum(xbuf[pl.ds(o, r), :].reshape(r // SUB, SUB, n), axis=0)
            acc = s if acc is None else acc + s
        b = [fold(acc[:, cb * LANES:(cb + 1) * LANES]) for cb in range(ncb)]
        bulk[0] = jnp.concatenate(b, axis=0)
        cps[0].start()

        t = [None] * ncb
        for cp in g_a:
            cp.wait()
        for cb in PAIR_A:
            t[cb] = fold(_tree_sum([tile(k, cb) for k in range(nt)]))
        tail_a[0] = jnp.concatenate([t[cb] for cb in PAIR_A], axis=0).astype(tail_a.dtype)
        cps[1].start()

        for cp in g_b0:
            cp.wait()
        part = {cb: _tree_sum([tile(k, cb) for k in range(nt - 1)]) for cb in PAIR_B}
        for cp in g_b1:
            cp.wait()
        for cb in PAIR_B:
            t[cb] = fold(part[cb] + tile(nt - 1, cb))
        tail_b[0] = jnp.concatenate([t[cb] for cb in PAIR_B], axis=0).astype(tail_b.dtype)
        cps[2].start()

        full[0] = jnp.concatenate([b[cb] + t[cb] for cb in range(ncb)], axis=0)
        cps[3].start()
        cps[4].start()
        for cp in cps:
            cp.wait_send()

        cps[3].wait_recv()
        cps[4].wait_recv()
        cps[0].wait_recv()
        out_ref[...] = (full[0] + full[1]) + (full[2] + bulk[1])
        pre = [out_ref[pl.ds(cb, 1), :] for cb in range(ncb)]
        for cp, buf, pair in ((cps[1], tail_a, PAIR_A), (cps[2], tail_b, PAIR_B)):
            cp.wait_recv()
            v = buf[1].astype(jnp.float32)
            for j, cb in enumerate(pair):
                out_ref[pl.ds(cb, 1), :] = pre[cb] + v[j:j + 1, :]

    out = pl.pallas_call(
        body,
        out_shape=jax.ShapeDtypeStruct((ncb, LANES), jnp.float32),
        in_specs=[pl.BlockSpec(memory_space=pl.ANY)],
        out_specs=pl.BlockSpec(memory_space=pltpu.VMEM),
        scratch_shapes=[
            pltpu.VMEM((m, n), jnp.float32),
            pltpu.VMEM((3, ncb, LANES), jnp.float32),
            pltpu.VMEM((2, ncb, LANES), jnp.float32),
            pltpu.VMEM((2, 2, LANES), jnp.bfloat16),
            pltpu.VMEM((2, 2, LANES), jnp.bfloat16),
            pltpu.SemaphoreType.DMA((5,)),
            pltpu.SemaphoreType.DMA((n_load,)),
            pltpu.SemaphoreType.DMA((5,)),
        ],
        compiler_params=_compiler_params(),
    )(x)
    return out.reshape(1, n)
```
